```python
import numpy as np
kernel_name = 'dist_attn_self_mha_htp_b1_sq256_skv256_d1024_hq8_dh128'

def setup_inputs():
    x = np.random.randn(1, 256, 1024).astype(np.float32)
    Wq = np.random.randn(1024, 4096).astype(np.float32) * 0.02
    Wk = np.random.randn(1024, 4096).astype(np.float32) * 0.02
    Wv = np.random.randn(1024, 4096).astype(np.float32) * 0.02
    Wo = np.random.randn(4096, 1024).astype(np.float32) * 0.02
    return {'x': x, 'Wq': Wq, 'Wk': Wk, 'Wv': Wv, 'Wo': Wo}

def reference(x, Wq, Wk, Wv, Wo):
    B, Sq, Hq, Hkv, Dh = (1, 256, 32, 32, 128)
    Q = (x @ Wq).reshape(B, Sq, Hq, Dh)
    K = (x @ Wk).reshape(B, Sq, Hkv, Dh)
    V = (x @ Wv).reshape(B, Sq, Hkv, Dh)
    Skv = K.shape[1]
    out = np.zeros((B, Sq, Hq, Dh), dtype=np.float32)
    m = np.full((B, Hq, Sq, 1), -np.inf, dtype=np.float32)
    l = np.zeros((B, Hq, Sq, 1), dtype=np.float32)
    for j0 in range(0, Skv, 256):
        Kj = K[:, j0:j0 + 256].copy()
        Vj = V[:, j0:j0 + 256].copy()
        sj = np.einsum('bihd,bjhd->bhij', Q, Kj).astype(np.float32) * 0.08838834764831843
        mj = sj.max(axis=-1, keepdims=True)
        m_new = np.maximum(m, mj)
        alpha = np.exp(m - m_new)
        pj = np.exp(sj - m_new)
        l = l * alpha + pj.sum(axis=-1, keepdims=True)
        out = out * alpha.transpose(0, 2, 1, 3) + np.einsum('bhij,bjhd->bihd', pj, Vj)
        m = m_new
    out = (out / l.transpose(0, 2, 1, 3)).reshape(B, Sq, Hq * Dh)
    return out @ Wo
```

```python
import contextlib
import jax
import jax.numpy as jnp
from jax import lax
from jax.experimental import pallas as pl
from jax.experimental.pallas import tpu as pltpu

bf = jnp.bfloat16
f32 = jnp.float32
S, D, H, DH = 256, 1024, 8, 128
SCALE = 0.08838834764831843
MESH = pl.DeviceIdType.MESH


def make(out_dtype=f32, scopes=False, lag2=2, lag3=4, prio3=0, wo_edges=(0, 128, 384, 640, 896, 1024),
         xshare=True, split0=True):
    NC = 8

    def scope(name):
        return jax.named_scope(name) if scopes else contextlib.nullcontext()

    def body(x_hbm, wq_hbm, wk_hbm, wv_hbm, wo_hbm, o_ref,
             xf, xh, wk, wq, wv, wo, kacc, qacc, vacc, kb, qb, pb, attn,
             sb1, rb1, keep, sb2, rb2, sb3, rb3,
             lsem, xs_sem, xr_sem, s1, r1, s2, r2, s3, r3):
        me = lax.axis_index("i")
        px = 3 - me
        py = me ^ 1
        cx = me >> 1
        cy = ((me + 1) >> 1) & 1
        offs = (0, 1, 3, 2)
        blk = [pl.multiple_of(((me + o) % 4) * 256, 256) for o in offs]

        loads = {}
        n = [0]
        def load(name, src, dst):
            c = pltpu.make_async_copy(src, dst, lsem.at[n[0]]); n[0] += 1
            c.start(); loads[name] = c
        if xshare:
            load("x", x_hbm.at[0, :, pl.ds(blk[0], 256)], xf.at[:, pl.ds(0, 256)])
        else:
            blk = [0, 256, 512, 768]
            load("x", x_hbm.at[0], xf)
        for s in range(4):
            load(f"k{s}", wk_hbm.at[pl.ds(blk[s], 256), :], wk.at[pl.ds(s * 256, 256), :])
            load(f"q{s}", wq_hbm.at[pl.ds(blk[s], 256), :], wq.at[pl.ds(s * 256, 256), :])
        for s in range(3):
            load(f"v{s}", wv_hbm.at[pl.ds(blk[s], 256), :], wv.at[pl.ds(s * 256, 256), :])
        load("v3a", wv_hbm.at[pl.ds(blk[3], 128), :], wv.at[pl.ds(768, 128), :])
        load("v3b", wv_hbm.at[pl.ds(blk[3] + 128, 128), :], wv.at[pl.ds(896, 128), :])
        for a, b in zip(wo_edges[:-1], wo_edges[1:]):
            load(f"o{a // 128}", wo_hbm.at[:, pl.ds(a, b - a)], wo.at[:, pl.ds(a, b - a)])

        bar = pltpu.get_barrier_semaphore()
        nbrs = (1, 3, 2) if xshare else (1, 3)
        for o in nbrs:
            pl.semaphore_signal(bar, inc=1, device_id=((me + o) % 4,), device_id_type=MESH)

        xsends = []
        with scope("x"):
            loads["x"].wait()
            if xshare:
                xh[0] = xf[:, 0:256].astype(bf)
            else:
                for s in range(4):
                    xh[s] = xf[:, s * 256:(s + 1) * 256].astype(bf)
        if xshare:
            with scope("bar"):
                pl.semaphore_wait(bar, len(nbrs))
                for s in (1, 2, 3):
                    c = pltpu.make_async_remote_copy(xh.at[0], xh.at[s], xs_sem.at[s], xr_sem.at[s],
                                                     device_id=((me + 4 - offs[s]) % 4,), device_id_type=MESH)
                    c.start(); xsends.append(c)

        rows = [pl.multiple_of((1 - cx) * 64, 64), pl.multiple_of(128 + (1 - cy) * 64, 64),
                pl.multiple_of(cx * 64, 64), pl.multiple_of(128 + cy * 64, 64)]

        def mm(a, b):
            return jnp.dot(a, b.astype(bf), preferred_element_type=f32)

        for s in range(4):
            with scope(f"k{s}"):
                if xshare and s > 0:
                    xsends[s - 1].wait_recv()
                loads[f"k{s}"].wait()
                d = mm(xh[s], wk[s * 256:(s + 1) * 256, :])
                if s == 0:
                    kacc[...] = d
                elif s < 3:
                    kacc[...] += d
                else:
                    kb[...] = (kacc[...] + d).astype(bf)
            with scope(f"q{s}"):
                loads[f"q{s}"].wait()
                d = mm(xh[s], wq[s * 256:(s + 1) * 256, :])
                if s == 0:
                    qacc[...] = d
                elif s < 3:
                    qacc[...] += d
                else:
                    qacc[...] = (qacc[...] + d) * SCALE
                    for r in range(4):
                        qb[r * 64:(r + 1) * 64, :] = qacc[pl.ds(rows[r], 64), :].astype(bf)

        def softmax(h):
            cs = slice(h * DH, (h + 1) * DH)
            s_ = lax.dot_general(qb[:, cs], kb[:, cs], (((1,), (1,)), ((), ())), preferred_element_type=f32)
            m = jnp.max(s_, axis=-1, keepdims=True)
            p = jnp.exp(s_ - m)
            l = jnp.sum(p, axis=-1, keepdims=True)
            pb[h] = (p * (1.0 / l)).astype(bf)

        with scope("sm"):
            for h in range(H):
                softmax(h)
        for s in range(3):
            with scope(f"v{s}"):
                loads[f"v{s}"].wait()
                d = mm(xh[s], wv[s * 256:(s + 1) * 256, :])
                if s == 0:
                    vacc[...] = d
                else:
                    vacc[...] += d
        with scope("v3a"):
            if not xshare:
                pl.semaphore_wait(bar, len(nbrs))
            loads["v3a"].wait()
            vacc[...] += mm(xh[3][:, 0:128], wv[768:896, :])
        with scope("v3b"):
            loads["v3b"].wait()
            kb[...] = (vacc[...] + mm(xh[3][:, 128:256], wv[896:1024, :])).astype(bf)
            if split0:
                for h in range(H):
                    cs = slice(h * DH, (h + 1) * DH)
                    attn[0:128, cs] = mm(pb[h, 0:128, :], kb[:, cs]).astype(bf)
            else:
                for h in range(H):
                    cs = slice(h * DH, (h + 1) * DH)
                    attn[:, cs] = mm(pb[h], kb[:, cs]).astype(bf)

        def rc(src, dst, ss, rs, dev):
            return pltpu.make_async_remote_copy(src, dst, ss, rs, device_id=(dev,), device_id_type=MESH)
        c1 = [[rc(sb1.at[j, t], rb1.at[j, t], s1.at[2 * j + t], r1.at[2 * j + t], (px, py)[t]) for t in range(2)] for j in range(NC)]
        c2 = [[rc(sb2.at[j, t], rb2.at[j, t], s2.at[2 * j + t], r2.at[2 * j + t], (py, px)[t]) for t in range(2)] for j in range(NC)]
        if out_dtype == bf:
            c3 = [[rc(o_ref.at[0, pl.ds(rows[2 + t], 64), pl.ds(j * 128, 128)], o_ref.at[0, pl.ds(rows[2 + t], 64), pl.ds(j * 128, 128)],
                      s3.at[2 * j + t], r3.at[2 * j + t], (px, py)[t]) for t in range(2)] for j in range(NC)]
        else:
            c3 = [[rc(sb3.at[j, t], rb3.at[j, t], s3.at[2 * j + t], r3.at[2 * j + t], (px, py)[t]) for t in range(2)] for j in range(NC)]

        def step1(j):
            with scope(f"a{j}"):
                if f"o{j}" in loads:
                    loads[f"o{j}"].wait()
                cs = slice(j * 128, (j + 1) * 128)
                if j == 0 and split0:
                    d = mm(attn[0:128, :], wo[:, cs])
                    sb1[j, 0] = d[0:64].astype(bf)
                    sb1[j, 1] = d[64:128].astype(bf)
                    c1[j][0].start(); c1[j][1].start()
                    for h in range(H):
                        hs = slice(h * DH, (h + 1) * DH)
                        attn[128:256, hs] = mm(pb[h, 128:256, :], kb[:, hs]).astype(bf)
                    keep[j] = mm(attn[128:256, :], wo[:, cs])
                else:
                    d = mm(attn[...], wo[:, cs])
                    sb1[j, 0] = d[0:64].astype(bf)
                    sb1[j, 1] = d[64:128].astype(bf)
                    keep[j] = d[128:256]
                    c1[j][0].start(); c1[j][1].start()

        def step2(j):
            with scope(f"b{j}"):
                for t in range(2):
                    c1[j][t].wait_recv()
                    v = keep[j, t * 64:(t + 1) * 64, :] + rb1[j, t].astype(f32)
                    keep[j, t * 64:(t + 1) * 64, :] = v
                    sb2[j, t] = v.astype(bf)
                    c2[j][t].start()

        def step3(j):
            with scope(f"c{j}"):
                for t in range(2):
                    c2[j][t].wait_recv()
                    v = keep[j, t * 64:(t + 1) * 64, :] + rb2[j, t].astype(f32)
                    o_ref[0, pl.ds(rows[2 + t], 64), j * 128:(j + 1) * 128] = v.astype(out_dtype)
                    if out_dtype != bf:
                        sb3[j, t] = v.astype(bf)
                    c3[j][t].start(priority=prio3)

        def step4(j):
            with scope(f"d{j}"):
                for t in range(2):
                    c3[j][t].wait_recv()
                    if out_dtype != bf:
                        o_ref[0, pl.ds(rows[t], 64), j * 128:(j + 1) * 128] = rb3[j, t].astype(out_dtype)

        for j in range(NC + lag3):
            if j < NC:
                step1(j)
            if 0 <= j - lag2 < NC:
                step2(j - lag2)
            if 0 <= j - lag3 < NC:
                step3(j - lag3)
        for j in range(NC):
            step4(j)
        with scope("fin"):
            for c in xsends:
                c.wait_send()
            for cc in (c1, c2, c3):
                for j in range(NC):
                    for t in range(2):
                        cc[j][t].wait_send()

    def fn(x, Wq, Wk, Wv, Wo):
        V = pltpu.VMEM
        DMA = pltpu.SemaphoreType.DMA
        return pl.pallas_call(
            body,
            out_shape=jax.ShapeDtypeStruct((1, S, D), out_dtype),
            in_specs=[pl.BlockSpec(memory_space=pl.ANY)] * 5,
            out_specs=pl.BlockSpec(memory_space=pltpu.VMEM),
            scratch_shapes=[
                V((S, D), f32), V((4, S, 256), bf),
                V((D, D), f32), V((D, D), f32), V((D, D), f32), V((D, D), f32),
                V((S, D), f32), V((S, D), f32), V((S, D), f32),
                V((S, D), bf), V((S, D), bf), V((H, S, S), bf), V((S, D), bf),
                V((NC, 2, 64, 128), bf), V((NC, 2, 64, 128), bf), V((NC, 128, 128), f32),
                V((NC, 2, 64, 128), bf), V((NC, 2, 64, 128), bf),
                V((NC, 2, 64, 128), bf), V((NC, 2, 64, 128), bf),
                DMA((24,)), DMA((4,)), DMA((4,)),
                DMA((2 * NC,)), DMA((2 * NC,)), DMA((2 * NC,)), DMA((2 * NC,)), DMA((2 * NC,)), DMA((2 * NC,)),
            ],
            compiler_params=pltpu.CompilerParams(
                collective_id=0, vmem_limit_bytes=48 << 20,
                disable_semaphore_checks=True, disable_bounds_checks=True),
        )(x, Wq, Wk, Wv, Wo)
    return fn


_fn = make()


def pallas_dist_attn_self_mha_htp_b1_sq256_skv256_d1024_hq8_dh128_kernel(x, Wq, Wk, Wv, Wo):
    return _fn(x, Wq, Wk, Wv, Wo)
```

```python
import jax
import jax.numpy as jnp
from jax import lax
from jax.experimental import pallas as pl
from jax.experimental.pallas import tpu as pltpu

bf = jnp.bfloat16
f32 = jnp.float32
S, D, H, DH = 256, 1024, 8, 128
SCALE = 0.08838834764831843
MESH = pl.DeviceIdType.MESH
NC = 8
PR = 32
NP = NC * S // PR

_PATH = {"a": (0, 1, 2, 3), "A": (0, 3, 2, 1), "b": (2, 1, 0, 3), "B": (2, 3, 0, 1),
         "Y": (0, 1, 2, 3), "y": (0, 3, 2, 1)}


def _msgs(kind):
    a, b, c, d = _PATH[kind]
    m = [(a, b, None), (b, c, 0), (c, d, 1), (d, c, None), (c, b, 3), (b, a, 4)]
    if kind in "Yy":
        m[2] = (a, d, 5)
    return m


def _fins(kind):
    a, b, c, d = _PATH[kind]
    return [(a, (5,), True), (b, (0, 4), True), (c, (1, 3), True), (d, (2,), kind not in "Yy")]


def _direction(src, dst):
    return 0 if dst == (src + 1) % 4 else 1


_SCHEDULE = """
types yBBAyyBBaYAaaYaaababbYbaAAyAByABYbbabBBBbbaababYAAaAAaayByAAABAy
ord 10623547,03472651,40235716,42501367
sw 11100101,00110100,10111001,01110010
prog0 | | | S12.0 | | | S9.0 S14.0 | | S15.0 S10.0 | S4.0 | S13.0 S5.0 | | | | S0.0 | S8.0 S11.0 |
+ S3.0 | S52.0 | | S54.0 | S55.0 | S48.0 S53.0 | | S50.0 S49.0 | S51.0 S1.4 | S16.0 | | S18.0 | S2.4
+ | | S21.0 | | S20.4 S22.4 S6.4 S17.4 S7.4 S23.0 | S24.0 | S25.0 | | S26.0 S19.4 | | | | | S27.0 |
+ S45.0 | | S47.0 S46.4 S28.4 S44.4 | S29.0 | | | S31.4 S41.4 S30.0 S43.0 S40.4 | | | | S42.0 S33.2
+ S32.2 | | | | S39.4 S32.0 | S60.0 | | | S34.4 S38.2 S62.0 S7.2 S38.4 | | S35.0 | | S58.0 S36.4
+ S59.0 S63.0 F20.2 S61.4 X12.0 X9.0 X10.0 X14.0 X15.0 X4.0 X13.0 X5.0 X0.0 X8.0 X3.0 X11.0 X52.0
+ X54.0 X55.0 X53.0 X48.0 X50.0 X49.0 X16.0 X51.0 X18.0 X1.4 X21.0 X2.4 X20.4 X6.4 X22.4 X7.4 X17.4
+ X24.0 X23.0 X25.0 X19.4 X26.0 X27.0 X45.0 X28.4 X47.0 X29.0 F3.0 S56.4 S20.2 X46.4 X31.4 X44.4
+ X30.0 X41.4 S21.2 S19.2 S1.2 X33.2 F28.2 S22.2 S4.2 S36.2 S0.2 S34.2 X43.0 X32.2 X40.4 X39.4 X42.0
+ X60.0 X32.0 X62.0 X34.4 X38.4 X38.2 F23.0 S37.4 F1.2 S33.4 F7.2 F38.2 S5.2 S6.2 X58.0 X7.2 X59.0
+ X35.0 X63.0 X36.4 S29.2 S37.2 S57.0 F5.0 S46.2 S26.2 F36.2 F46.2 S40.2 X61.4 X1.2 X56.4 X4.2 X20.2
+ X0.2 S57.2 F6.2 F25.0 S44.2 X21.2 X33.4 S56.2 S47.2 F19.2 S2.2 F16.0 X19.2 X5.2 X22.2 X6.2 S63.2
+ S61.2 X36.2 X29.2 X34.2 X37.2 F14.0 S28.2 S31.2 F57.0 F21.0 S41.2 F39.2 F56.2 S17.2 F58.0 F18.0
+ F17.2 F32.0 X37.4 X26.2 X57.0 X57.2 F9.0 X46.2 X56.2 S13.2 S55.2 F27.0 F26.0 F47.0 F0.0 F30.0
+ F33.2 F44.2 F41.2 S9.2 F62.0 F31.2 S39.2 F37.2 F34.2 F2.2 F35.0 F22.2 F4.0 F24.0 F29.0 F40.2 F42.0
+ F43.0 F61.2 F45.0 F63.0 F8.0 F60.0 F11.0 F59.0 F15.0 F55.0 F13.0 F52.0 F53.0 F48.0 F54.0 X40.2
+ X2.2 X44.2 X63.2 X47.2 X61.2 X41.2 X28.2 X17.2 X31.2 F51.0 F12.0 X13.2 X55.2 F49.0 F50.0 X9.2
+ X39.2 F10.0
prog1 | S0.3 | | | S1.3 S3.3 | | S5.3 S2.3 | | S4.3 | S6.3 | | S25.3 | S26.3 S7.3 | S28.3 | | S30.3
+ | S29.3 S31.3 S24.3 | | S37.3 S27.3 | S38.3 | | | S39.3 | | S36.1 | S60.3 | S61.3 | S62.3 | S34.1
+ S63.3 S33.1 | | | | S57.3 S32.5 S58.3 S56.3 S59.3 | | | | S35.5 S16.1 | | | | S20.1 S21.1 S22.1
+ S18.1 | | S52.3 | | S19.1 S55.3 S17.1 | | | S48.3 | S51.3 S49.3 S21.5 S50.1 S18.5 F17.1 S54.1 | |
+ | | S16.5 S23.5 | | | | S44.1 S45.1 S46.1 | | | | S10.3 S40.1 S53.1 S11.1 S47.5 | | | | S41.1
+ S42.5 S8.1 S23.1 X0.3 X1.3 X3.3 X2.3 X5.3 X4.3 X6.3 X25.3 X7.3 X26.3 X28.3 X30.3 X31.3 X29.3 X37.3
+ X24.3 X38.3 X27.3 X39.3 X36.1 X60.3 X61.3 X62.3 X34.1 X63.3 X33.1 X57.3 X32.5 X58.3 S43.5 S15.1
+ S12.1 F40.1 X56.3 X59.3 X35.5 X16.1 X20.1 X21.1 X22.1 X18.1 X19.1 X52.3 X17.1 X55.3 X21.5 X48.3
+ X18.5 X51.3 X16.5 X49.3 X23.5 X50.1 X44.1 X54.1 X46.1 X45.1 X40.1 X10.3 S45.5 F21.1 S43.1 S40.5
+ X47.5 X53.1 S8.5 S42.1 X41.1 X11.1 S11.5 F44.1 X42.5 X8.1 S14.5 X43.5 X23.1 S15.5 X45.5 X15.1
+ S36.5 S35.1 F8.1 S9.5 F35.1 S14.1 S34.5 F14.1 F45.1 S47.1 F34.1 F15.1 X8.5 X12.1 S13.5 S20.5 S13.1
+ X11.5 X43.1 S53.5 F1.3 S44.5 S32.1 S46.5 F7.3 F23.1 S17.5 X14.5 X40.5 S54.5 F32.1 X15.5 X42.1
+ S12.5 F53.1 X9.5 X36.5 S50.5 F22.1 F41.1 F54.1 X13.5 X35.1 X53.5 X14.1 X54.5 X34.5 X12.5 X47.1
+ F10.3 S41.5 S19.5 F26.3 F12.1 X50.5 X20.5 X13.1 X44.5 X32.1 F63.3 F2.3 F49.3 F19.1 F38.3 F56.3
+ F20.1 S9.1 S22.5 F29.3 S33.5 F18.1 F16.1 F46.1 F47.1 F43.1 F42.1 F3.3 F11.1 F36.1 F9.1 F13.1 F4.3
+ F0.3 F33.1 F5.3 F50.1 F6.3 F24.3 F27.3 F37.3 F25.3 F57.3 F30.3 F52.3 F62.3 F61.3 F48.3 F28.3 X46.5
+ X17.5 X41.5 F51.3 X19.5 F31.3 X9.1 F60.3 F55.3 X22.5 F58.3 F39.3 X33.5 F59.3
prog2 | | S37.0 | S38.0 S36.0 | | | S33.0 | S34.0 S39.0 | | | S1.0 | | S2.0 S32.4 S0.4 | | | | S7.0
+ S35.4 S6.0 | S20.0 | | | S5.4 S3.4 S22.0 | | S17.0 | | S19.0 S21.4 S4.4 | S28.0 | | | S31.0 S18.4
+ S30.4 S16.4 | | | | S23.4 S24.4 S26.4 | S44.0 | | | S46.0 S47.4 S29.4 S25.4 | S40.0 | | | S41.0
+ S42.4 S43.4 S27.4 | S56.0 | | | S3.2 S57.4 | | S61.0 | | S58.4 S45.4 S63.4 S60.4 | | | | S8.4
+ S59.4 S18.2 S62.4 S11.4 F21.2 | | | | S14.4 S15.4 S9.4 | | | | S55.4 S52.4 S13.4 | | | | S53.4
+ S48.4 F5.2 S51.4 S49.4 X37.0 X36.0 X38.0 X33.0 X39.0 X34.0 X1.0 X32.4 X2.0 X0.4 X35.4 X7.0 X20.0
+ S54.4 X6.0 X22.0 X5.4 X17.0 X3.4 X19.0 X4.4 X21.4 X28.0 X18.4 X31.0 F54.2 S12.4 X16.4 X30.4 X23.4
+ X24.4 X44.0 X26.4 X46.0 X29.4 X47.4 X25.4 X40.0 X27.4 X41.0 X56.0 X42.4 X57.4 X43.4 X61.0 X3.2
+ X58.4 X45.4 X63.4 X8.4 X60.4 X11.4 X59.4 X14.4 X18.2 X15.4 X62.4 X9.4 X55.4 S50.4 S10.4 S45.2
+ S24.2 F3.2 S16.2 S27.2 F0.2 F10.2 S25.2 S50.2 F18.2 S53.2 S10.2 X13.4 X52.4 X53.4 X48.4 X54.4
+ X51.4 X12.4 X49.4 S30.2 X50.4 X10.4 S15.2 F49.2 S49.2 S11.2 F23.2 X24.2 X45.2 X27.2 X16.2 S52.2
+ F52.2 F50.2 S12.2 F16.2 F27.2 X25.2 X50.2 S62.2 S48.2 S8.2 F15.2 S51.2 X10.2 X53.2 S60.2 S54.2
+ S43.2 F60.2 X30.2 X15.2 X49.2 X11.2 S58.2 S35.2 F24.2 F30.2 X52.2 X12.2 S14.2 X62.2 X8.2 S59.2
+ S23.2 F11.2 F34.0 F12.2 X48.2 X54.2 F38.0 F62.2 F48.2 S42.2 F4.2 F25.2 F45.2 F53.2 F51.2 F8.2
+ F31.0 F43.2 F40.0 F42.2 F39.0 F36.0 F58.2 F35.2 F26.2 F14.2 F59.2 F47.2 F1.0 X51.2 X43.2 X60.2
+ X35.2 X58.2 X14.2 F20.0 X59.2 F7.0 X23.2 F13.2 F61.0 X42.2 F44.0 F63.2 F32.2 F6.0 F46.0 F28.0
+ F17.0 F29.2 F41.0 F57.2 F19.0 F37.0 F9.2 F56.0 F22.0 F2.0 F33.0 F55.2
prog3 | S32.3 | S33.3 | S34.3 | | S36.3 | S35.3 | | | S20.3 | S21.3 | S22.3 | S23.3 | | S17.3 S16.3
+ | S18.3 | S19.3 | S44.3 | S45.3 | S46.3 | S47.3 | S40.3 | | S42.3 | S43.3 S37.1 S41.3 | | | | S4.1
+ S39.1 S38.1 S5.1 | | | | S3.1 S1.1 S0.1 S2.1 | S8.3 | | | S0.5 S11.3 S10.1 S7.1 F0.1 | | | | S15.3
+ S14.3 S6.1 S5.5 | | | S9.3 | S4.5 S13.3 S3.5 S12.3 | | | | S24.1 S28.1 S31.1 | | | S53.3 S54.3 |
+ S30.5 S26.5 S25.1 S24.5 | | | | S50.3 S29.5 F26.1 S25.5 S27.1 | | | | S51.1 S49.1 S27.5 S30.1
+ S57.5 S48.1 F4.1 S56.1 F1.1 | | | | S61.1 S31.5 S52.1 X32.3 X33.3 X34.3 X35.3 X36.3 X20.3 X21.3
+ X22.3 X23.3 X17.3 X16.3 X19.3 X18.3 X44.3 X45.3 X46.3 X47.3 X40.3 X42.3 X37.1 X43.3 X41.3 X4.1
+ X39.1 X5.1 X38.1 X3.1 X1.1 X0.1 X2.1 S63.5 X8.3 X0.5 X11.3 X7.1 X10.1 X6.1 X15.3 X5.5 X14.3 X4.5
+ X9.3 X3.5 X13.3 X28.1 X12.3 X31.1 X24.1 X30.5 X53.3 X26.5 X54.3 X24.5 X25.1 X29.5 X50.3 X25.5
+ X27.1 X27.5 X51.1 S60.5 S62.1 S60.1 S58.5 X57.5 X49.1 S59.5 S39.5 S58.1 S26.1 X56.1 X30.1 X61.1
+ X48.1 S62.5 S59.1 F59.1 F38.1 X63.5 X31.5 S55.5 S38.5 X60.5 X52.1 S52.5 S1.5 S7.5 F61.1 F29.1
+ F25.1 S61.5 F5.1 X58.5 X62.1 S48.5 X59.5 X60.1 S51.5 X62.5 X39.5 S49.5 X55.5 X58.1 S10.5 F27.1
+ S63.1 F6.1 F39.1 S6.5 S28.5 X52.5 X26.1 X48.5 X59.1 X51.5 X38.5 X49.5 X1.5 F57.1 F16.3 S29.1 S57.1
+ F30.1 S37.5 X10.5 X7.5 X61.5 X63.1 F44.3 F36.3 S56.5 X6.5 F8.3 F28.1 F60.1 F21.3 F10.1 F18.3 F24.1
+ F11.3 F45.3 F48.1 S2.5 F55.1 F50.3 F52.1 X28.5 F41.3 F47.3 F51.1 F54.3 F34.3 F15.3 F3.1 F40.3
+ S55.1 F2.1 F7.1 F31.1 F33.3 F32.3 F58.1 F62.1 F63.1 F56.1 F20.3 F49.1 F19.3 F22.3 F37.1 F53.3
+ F46.3 F12.3 F43.3 F17.3 F35.3 X29.1 X57.1 X37.5 X56.5 F13.3 F14.3 X2.5 F9.3 F23.3 X55.1 F42.3
"""

_XORD = [[1, 2, 3, 0], [1, 0, 3, 2], [0, 1, 2, 3], [2, 0, 3, 1]]
_XACT = [
    "s1a>1 s2a>3 s1b>1 s2b>3 s3a>1 s3b>3 s3b>1 s3a>3 s2b>1 s1b>3 | | | w0a w0b",
    "s0a>2 s0a>0 w1a s1a>2 w1b s1b>2 | w3a s3a>2 w0b | w3b | w2a w2b",
    "w0a s0a>3 w0b s0b>1 | w1a s1a>3 w2a s2a>1 w1b | w2b | w3a w3b",
    "s0b>2 s0b>0 w2a s2a>2 w2b s2b>2 | w3b s3b>2 w0a | w3a | w1a w1b",
]
_XACT = [[step.split() for step in acts.split("|")] for acts in _XACT]
_XSENDS = [[a for step in acts for a in step if a[0] == "s"] for acts in _XACT]

_VGROUPS = [[(0, 0, 256), (0, 256, 256)], [(0, 512, 256)], [(0, 768, 256)],
            [(1, 0, 256)], [(1, 256, 256)],
            [(1, 512, 128)], [(1, 640, 128)], [(1, 768, 128)], [(1, 896, 128)]]
_VLOADS = [v for g in _VGROUPS for v in g]

_KSEM, _K3SEM, _XSEM, _OSEM, _VSEM = 0, 6, 10, 11, 19


def _parse(text):
    f = {}
    for line in text.replace("\n+ ", " ").strip().split("\n"):
        key, val = line.split(" ", 1)
        f[key] = val
    order = [[int(c) for c in o] for o in f["ord"].split(",")]
    sw = [[int(c) for c in o] for o in f["sw"].split(",")]
    types, segs = f["types"], []
    for chip in range(4):
        waited, prog = set(), []
        for seg in f["prog%d" % chip].split("|"):
            ops = []
            for op in seg.split():
                p, i = (int(v) for v in op[1:].split("."))
                need = {"W": (i,), "X": (), "F": _fins(types[p])[i % 4][1],
                        "S": [q for q in _msgs(types[p])[i][2:] if q is not None]}[op[0]]
                for q in need:
                    if (p, q) not in waited:
                        waited.add((p, q))
                        ops.append(("W", p, q))
                if op[0] != "W":
                    ops.append((op[0], p, i))
            prog.append(ops)
        flat = sorted(op for ops in prog for op in ops)
        want = [("F", p, i) for p in range(NP) for i, fin in enumerate(_fins(types[p])) if fin[0] == chip]
        for kind, end in (("S", 0), ("W", 1), ("X", 0)):
            want += [(kind, p, i) for p in range(NP) for i, m in enumerate(_msgs(types[p])) if m[end] == chip]
        assert len(prog) == NP + 1 and flat == want
        segs.append(prog)
    return types, order, sw, segs


_TYPES, _ORDER, _SW, _SEGS = _parse(_SCHEDULE)


def _body(x_hbm, wq_hbm, wk_hbm, wv_hbm, wo_hbm, o_ref,
          xf, xh, wkq, wkq3, wv, wo, acc, vacc, kb, qb, pb, attn, part, sbuf, rbuf,
          lsem, xs_sem, xr_sem, ssem, rsem):
    me = lax.axis_index("i")

    def table(rows, bits):
        codes = [sum(v << (bits * k) for k, v in enumerate(r)) for r in rows]
        code = jnp.where(me < 2, jnp.where(me == 0, codes[0], codes[1]),
                         jnp.where(me == 2, codes[2], codes[3]))
        return lambda k: (code >> (bits * k)) & ((1 << bits) - 1)

    def by_chip(f):
        lax.cond((me & 1) == 1,
                 lambda: lax.cond(me == 1, lambda: f(1), lambda: f(3)),
                 lambda: lax.cond(me == 2, lambda: f(2), lambda: f(0)))

    def load(src, dst, sem):
        pltpu.make_async_copy(src, dst, lsem.at[sem]).start()

    def load2(src, dst, sem):
        for i in range(2):
            load(src.at[:, pl.ds(16 * i, 16), :], dst.at[:, pl.ds(16 * i, 16), :], sem)

    def wait_load(dst, sem):
        pltpu.make_async_copy(dst, dst, lsem.at[sem]).wait()

    def mm(a, b):
        return jnp.dot(a, b.astype(bf), preferred_element_type=f32)

    def xload(half):
        for i in range(4):
            load(x_hbm.at[pl.ds(4 * half, 4), pl.ds(8 * i, 8), pl.ds(0, 256)],
                 xf.at[pl.ds(0, 4), pl.ds(8 * i, 8), pl.ds(0, 256)], _XSEM)

    pl.when(me == 3)(lambda: xload(1))
    pl.when(me == 1)(lambda: xload(0))

    @pl.when(me == 0)
    def _():
        load(x_hbm.at[:, :, pl.ds(256, 768)], xf, _XSEM)

    xblock = table(_XORD, 2)
    for s in range(3):
        for w, w_hbm in enumerate((wk_hbm, wq_hbm)):
            load(w_hbm.at[pl.ds(xblock(s) * 8, 8)], wkq.at[2 * s + w], _KSEM + 2 * s + w)
    for hf in range(2):
        for w, w_hbm in enumerate((wk_hbm, wq_hbm)):
            load2(w_hbm.at[pl.ds(xblock(3) * 8, 8), :, pl.ds(hf * 512, 512)],
                  wkq3.at[2 * hf + w], _K3SEM + 2 * hf + w)

    barrier = pltpu.get_barrier_semaphore()
    for o in (1, 3):
        pl.semaphore_signal(barrier, inc=1, device_id=((me + o) & 3,), device_id_type=MESH)

    def xunit(chip, name):
        slot, hf = _XORD[chip].index(int(name[0])), "ab".index(name[1])
        return xh.at[slot, pl.ds(128 * hf, 128)], xr_sem.at[2 * slot + hf]

    def xsend(chip, act):
        name, dst = act[1:].split(">")
        dst_ref, dst_sem = xunit(int(dst), name)
        return pltpu.make_async_remote_copy(
            xunit(chip, name)[0], dst_ref, xs_sem.at[_XSENDS[chip].index(act)], dst_sem,
            device_id=(int(dst),), device_id_type=MESH)

    def xcast(chip):
        if chip == 0:
            wait_load(xf, _XSEM)
            for k in range(3):
                xh[k] = xf[:, :, 256 * k:256 * (k + 1)].reshape(S, 256).astype(bf)
        elif chip != 2:
            wait_load(xf.at[pl.ds(0, 4), :, pl.ds(0, 256)], _XSEM)
            r0 = 128 * (chip >> 1)
            xh[1, r0:r0 + 128] = xf[0:4, :, 0:256].reshape(128, 256).astype(bf)

    def xstep(step):
        def run(chip):
            for act in _XACT[chip][step]:
                if act[0] == "s":
                    xsend(chip, act).start()
                else:
                    ref, sem = xunit(chip, act[1:])
                    pltpu.make_async_remote_copy(ref, ref, xs_sem.at[0], sem, device_id=(chip,),
                                                 device_id_type=MESH).wait_recv()
        by_chip(run)

    def xdone(chip):
        for act in _XSENDS[chip]:
            xsend(chip, act).wait_send()

    acc[...] = jnp.zeros_like(acc)
    by_chip(xcast)
    pl.semaphore_wait(barrier, 2)
    xstep(0)

    def kq(t, carry):
        pl.when(t == 2)(lambda: xstep(1))
        pl.when(t == 4)(lambda: xstep(2))
        wait_load(wkq.at[t], _KSEM + t)
        d = mm(xh[t >> 1], wkq[t].reshape(256, D))
        for hf in range(2):
            acc[2 * hf + (t & 1)] += d[:, hf * 512:(hf + 1) * 512]
        return carry

    lax.fori_loop(0, 6, kq, 0)

    def vdst(v):
        hf, r0, rn = v
        return wv.at[hf, pl.ds(r0 // 32, rn // 32)]

    for n, v in enumerate(_VLOADS):
        load2(wv_hbm.at[pl.ds(v[1] // 32, v[2] // 32), :, pl.ds(v[0] * 512, 512)], vdst(v), _VSEM + n)
    xstep(3)
    by_chip(xdone)

    def kq3(hf, carry):
        wait_load(wkq3.at[2 * hf], _K3SEM + 2 * hf)
        kb[...] = (acc[2 * hf] + mm(xh[3], wkq3[2 * hf].reshape(256, 512))).astype(bf)
        wait_load(wkq3.at[2 * hf + 1], _K3SEM + 2 * hf + 1)
        qb[...] = ((acc[2 * hf + 1] + mm(xh[3], wkq3[2 * hf + 1].reshape(256, 512))) * SCALE).astype(bf)
        for hh in range(4):
            cs = slice(hh * DH, (hh + 1) * DH)
            s = lax.dot_general(qb[:, cs], kb[:, cs], (((1,), (1,)), ((), ())),
                                preferred_element_type=f32)
            p = jnp.exp(s - jnp.max(s, axis=-1, keepdims=True))
            pb[4 * hf + hh] = (p * (1.0 / jnp.sum(p, axis=-1, keepdims=True))).astype(bf)
        return carry

    lax.fori_loop(0, 2, kq3, 0)

    chunk = table(_ORDER, 3)

    def wo_start(slot):
        col = pl.multiple_of(chunk(slot) * 128, 128)
        nk = 2 if slot < 4 else 1
        for kh in range(nk):
            gs = pl.ds(32 // nk * kh, 32 // nk)
            load2(wo_hbm.at[gs, :, pl.ds(col, 128)], wo.at[slot, gs], _OSEM + slot)

    xslot = table([[o.index(b) for b in range(4)] for o in _XORD], 2)
    for gi, group in enumerate(_VGROUPS):
        if gi in (2, 4):
            for slot in range(2 * gi - 4, 2 * gi):
                wo_start(slot)
        for v in group:
            wait_load(vdst(v), _VSEM + _VLOADS.index(v))
        hf = group[0][0]

        def vpart(rs, cs):
            d = None if group[0][1] == 0 else vacc[rs, cs]
            for _, r0, rn in group:
                w = wv[hf, r0 // 32:(r0 + rn) // 32, :, cs]
                t = mm(xh[xslot(r0 // 256), rs, r0 % 256:r0 % 256 + rn], w.reshape(rn, w.shape[-1]))
                d = t if d is None else d + t
            return d

        if group[-1][1] + group[-1][2] < D:
            vacc[...] = vpart(slice(None), slice(None))
            continue
        if group[-1][2] == 128:
            vv = jnp.concatenate([
                jnp.concatenate([vpart(slice(mh * 128, (mh + 1) * 128),
                                       slice(hp * 256, (hp + 1) * 256)).astype(bf)
                                 for mh in range(2)], axis=0) for hp in range(2)], axis=1)
        else:
            vv = vpart(slice(None), slice(None)).astype(bf)
        for hh in range(4):
            h = hf * 4 + hh
            attn[:, h * DH:(h + 1) * DH] = mm(pb[h], vv[:, hh * DH:(hh + 1) * DH]).astype(bf)

    def segment(chip, ops):
        def copy(p, i):
            src, dst, dep = _msgs(_TYPES[p])[i]
            dr = _direction(src, dst)
            rows = pl.ds(PR * (p % 8), PR)
            return pltpu.make_async_remote_copy(
                sbuf.at[2 if dep is None else dr, _ORDER[chip].index(p // 8), rows],
                rbuf.at[dr * NC + p // 8, rows], ssem.at[dr * NP + p], rsem.at[dr * NP + p],
                device_id=(dst,), device_id_type=MESH)

        def payload(p, i):
            src, dst, _ = _msgs(_TYPES[p])[i]
            return rbuf[_direction(src, dst) * NC + p // 8, pl.ds(PR * (p % 8), PR)].astype(f32)

        for kind, p, i in ops:
            j, slot, rows = p // 8, _ORDER[chip].index(p // 8), pl.ds(PR * (p % 8), PR)
            if kind == "S":
                src, dst, dep = _msgs(_TYPES[p])[i]
                assert src == chip
                if dep is not None:
                    sbuf[_direction(src, dst), slot, rows] = (part[slot, rows] + payload(p, dep)).astype(bf)
                copy(p, i).start()
            elif kind == "W":
                copy(p, i).wait_recv()
            elif kind == "X":
                copy(p, i).wait_send()
            else:
                who, incoming, own = _fins(_TYPES[p])[i]
                assert who == chip
                vals = [payload(p, q) for q in incoming]
                v = part[slot, rows] + vals[0] if own else vals[0]
                for r in vals[1:]:
                    v = v + r
                o_ref[0, rows, j * 128:(j + 1) * 128] = v

    def run_segment(k):
        if any(_SEGS[chip][k] for chip in range(4)):
            by_chip(lambda chip: segment(chip, _SEGS[chip][k]))

    first_half = table(_SW, 1)
    run_segment(0)
    for blk in range(2 * NC):
        slot, b = blk >> 1, blk & 1
        if len({_SW[chip][slot] for chip in range(4)}) == 1:
            def rows(off, n, row0=(b ^ _SW[0][slot]) * 128):
                return pl.ds(row0 + off, n)
        else:
            def rows(off, n, row0=(first_half(slot) ^ b) * 128):
                return pl.ds(pl.multiple_of(row0 + off, n), n)
        if b == 0:
            wait_load(wo.at[slot], _OSEM + slot)
        d = jnp.concatenate([mm(attn[rows(64 * e, 64), :], wo[slot].reshape(D, 128))
                             for e in range(2)], axis=0)
        for q in range(4):
            dq = d[PR * q:PR * (q + 1)]
            part[slot, rows(PR * q, PR)] = dq
            sbuf[2, slot, rows(PR * q, PR)] = dq.astype(bf)
            run_segment(4 * blk + q + 1)


def pallas_dist_attn_self_mha_htp_b1_sq256_skv256_d1024_hq8_dh128_kernel(
    x: jax.Array,
    Wq: jax.Array,
    Wk: jax.Array,
    Wv: jax.Array,
    Wo: jax.Array,
):
    vmem = pltpu.VMEM
    dma = pltpu.SemaphoreType.DMA
    return pl.pallas_call(
        _body,
        out_shape=jax.ShapeDtypeStruct((1, S, D), f32),
        in_specs=[pl.BlockSpec(memory_space=pl.ANY)] * 5,
        out_specs=pl.BlockSpec(memory_space=pltpu.VMEM),
        scratch_shapes=[
            vmem((8, 32, 768), f32),
            vmem((4, S, 256), bf),
            vmem((6, 8, 32, D), f32),
            vmem((4, 8, 32, 512), f32),
            vmem((2, 32, 32, 512), f32),
            vmem((NC, 32, 32, 128), f32),
            vmem((4, S, 512), f32),
            vmem((S, 512), f32),
            vmem((S, 512), bf),
            vmem((S, 512), bf),
            vmem((H, S, S), bf),
            vmem((S, D), bf),
            vmem((NC, S, 128), f32),
            vmem((3, NC, S, 128), bf),
            vmem((2 * NC, S, 128), bf),
            dma((_VSEM + len(_VLOADS),)), dma((10,)), dma((8,)),
            dma((2 * NP,)), dma((2 * NP,)),
        ],
        compiler_params=pltpu.CompilerParams(
            collective_id=0, vmem_limit_bytes=48 << 20, disable_semaphore_checks=True),
    )(x.reshape(8, 32, D), Wq.reshape(32, 32, D), Wk.reshape(32, 32, D),
      Wv.reshape(32, 32, D), Wo.reshape(32, 32, D))
```
